```python
import numpy as np

kernel_name = "dist_rmsnorm_colshard_i_m768_n512"

def setup_inputs():
    x = np.random.randn(768, 2048).astype(np.float32)
    gamma = np.random.randn(2048).astype(np.float32)
    return {"x": x, "gamma": gamma}

def reference(x: np.ndarray, gamma: np.ndarray) -> np.ndarray:
    eps = 1e-5
    rms = np.sqrt(np.mean(x * x, axis=1, keepdims=True) + eps)
    return gamma * x / rms
```

```python
import jax
import jax.numpy as jnp
from jax import lax
from jax.experimental import pallas as pl
from jax.experimental.pallas import tpu as pltpu

N_DEV = 4
EPS = 1e-5
SUBLANES, LANES = 8, 128
NEAR = (1, 3)
FAR = 2

HEAD = (256, 256)
TAIL = (128, 80, 48)


def pallas_dist_rmsnorm_colshard_i_m768_n512_kernel(
    x: jax.Array,
    gamma: jax.Array,
):
    m, n = x.shape
    n_head, n_tail = sum(HEAD), len(TAIL)
    chunk_rows = HEAD + TAIL
    chunk_start = [sum(chunk_rows[:k]) for k in range(len(chunk_rows))]
    tail_start = chunk_start[len(HEAD):]
    assert sum(chunk_rows) == m and n % LANES == 0
    assert all(r % LANES == 0 for r in HEAD)
    assert all(r % SUBLANES == 0 and r <= LANES for r in TAIL)
    inv_cols = 1.0 / (n * N_DEV)
    tile = (SUBLANES, LANES)

    def body(
        x_hbm, g_hbm, out,
        xv, gv, head_own, head_in, tail_own, tail_near, tail_far, tail_base,
        load_sems, g_sem, send_sems, head_sem, near_sem, far_sems,
    ):
        loads = []
        for k, (r0, rows) in enumerate(zip(chunk_start, chunk_rows)):
            chunk = pl.ds(r0, rows)
            loads.append(
                pltpu.make_async_copy(x_hbm.at[chunk], xv.at[chunk], load_sems.at[k])
            )
            loads[-1].start()

        me = lax.axis_index("i")

        def peer(dist):
            return dict(
                device_id=((me + dist) & (N_DEV - 1),),
                device_id_type=pl.DeviceIdType.MESH,
            )

        barrier = pltpu.get_barrier_semaphore()
        for dist in (FAR, *NEAR):
            pl.semaphore_signal(barrier, 1, **peer(dist))

        g_load = pltpu.make_async_copy(g_hbm, gv, g_sem)
        g_load.start()

        sends = []

        def send(src, dst, recv_sem, dist):
            sends.append(
                pltpu.make_async_remote_copy(
                    src, dst, send_sems.at[len(sends)], recv_sem, **peer(dist)
                )
            )
            sends[-1].start()

        sub = lax.broadcasted_iota(jnp.int32, tile, 0)
        skew = lax.broadcasted_iota(jnp.int32, tile, 1) - sub

        def packed_sumsq(r0, rows):
            acc = jnp.zeros(tile, jnp.float32)
            for l in range(0, rows, SUBLANES):
                v = xv[pl.ds(r0 + l, SUBLANES), :]
                v = v * v
                parts = [v[:, c : c + LANES] for c in range(0, n, LANES)]
                while len(parts) > 1:
                    parts = [sum(parts[i + 1 : i + 2], parts[i]) for i in range(0, len(parts), 2)]
                row_sum = jnp.sum(parts[0], axis=1, keepdims=True)
                acc = jnp.where(skew == l, row_sum, acc)
            return jnp.sum(acc, axis=0, keepdims=True)

        def unpack(packed, l):
            return jnp.sum(jnp.where(skew == l, packed, 0.0), axis=1, keepdims=True)

        def to_tile(v):
            return jnp.broadcast_to(v, tile)

        for k, rows in enumerate(HEAD):
            loads[k].wait()
            for r0 in range(chunk_start[k], chunk_start[k] + rows, LANES):
                head_own[pl.ds(r0 // LANES, 1), :] = packed_sumsq(r0, LANES)
        pl.semaphore_wait(barrier, N_DEV - 1)
        for dist in (FAR, *NEAR):
            send(head_own, head_in.at[dist - 1], head_sem, dist)
        for t, rows in enumerate(TAIL):
            loads[len(HEAD) + t].wait()
            tail_own[t] = packed_sumsq(tail_start[t], rows)
            send(tail_own.at[t], tail_far.at[t], far_sems.at[t], FAR)
        for slot, dist in enumerate(NEAR):
            send(tail_own, tail_near.at[slot], near_sem, dist)

        g_load.wait()
        g = jnp.broadcast_to(gv[...].reshape(1, n), (SUBLANES, n))
        for r0 in range(0, m, SUBLANES):
            xv[pl.ds(r0, SUBLANES), :] = xv[pl.ds(r0, SUBLANES), :] * g
        for copy in sends:
            copy.wait_send()

        pltpu.make_async_copy(tail_near, tail_near, near_sem).wait()
        for t, rows in enumerate(TAIL):
            total = to_tile(tail_own[t]) + (
                to_tile(tail_near[0, t]) + to_tile(tail_near[1, t])
            )
            for l in range(0, rows, SUBLANES):
                group = (tail_start[t] - n_head + l) // SUBLANES
                tail_base[group] = to_tile(unpack(total, l))

        pltpu.make_async_copy(head_in, head_in, head_sem).wait()
        for r0 in range(0, n_head, LANES):
            line = pl.ds(r0 // LANES, 1)
            total = (to_tile(head_own[line, :]) + to_tile(head_in[0, line, :])) + (
                to_tile(head_in[1, line, :]) + to_tile(head_in[2, line, :])
            )
            scale = lax.rsqrt(total * inv_cols + EPS)
            for l in range(0, LANES, SUBLANES):
                rows8 = pl.ds(r0 + l, SUBLANES)
                out[rows8, :] = xv[rows8, :] * unpack(scale, l)

        for t, rows in enumerate(TAIL):
            pltpu.make_async_copy(tail_far.at[t], tail_far.at[t], far_sems.at[t]).wait()
            for l in range(0, rows, SUBLANES):
                far = jnp.full(tile, tail_far[t, 0, l], jnp.float32)
                for i in range(1, SUBLANES):
                    far = jnp.where(sub == i, tail_far[t, 0, l + i], far)
                group = (tail_start[t] - n_head + l) // SUBLANES
                scale = lax.rsqrt((tail_base[group] + far) * inv_cols + EPS)
                rows8 = pl.ds(tail_start[t] + l, SUBLANES)
                out[rows8, :] = xv[rows8, :] * jnp.tile(scale, (1, n // LANES))

    f32 = jnp.float32
    return pl.pallas_call(
        body,
        out_shape=jax.ShapeDtypeStruct((m, n), x.dtype),
        in_specs=[pl.BlockSpec(memory_space=pltpu.HBM)] * 2,
        out_specs=pl.BlockSpec(memory_space=pltpu.VMEM),
        scratch_shapes=[
            pltpu.VMEM((m, n), f32),
            pltpu.VMEM((n,), f32),
            pltpu.VMEM((n_head // LANES, LANES), f32),
            pltpu.VMEM((N_DEV - 1, n_head // LANES, LANES), f32),
            pltpu.VMEM((n_tail, 1, LANES), f32),
            pltpu.VMEM((len(NEAR), n_tail, 1, LANES), f32),
            pltpu.SMEM((n_tail, 1, LANES), f32),
            pltpu.VMEM((sum(TAIL) // SUBLANES, *tile), f32),
            pltpu.SemaphoreType.DMA((len(chunk_rows),)),
            pltpu.SemaphoreType.DMA,
            pltpu.SemaphoreType.DMA((N_DEV - 1 + n_tail + len(NEAR),)),
            pltpu.SemaphoreType.DMA,
            pltpu.SemaphoreType.DMA,
            pltpu.SemaphoreType.DMA((n_tail,)),
        ],
        compiler_params=pltpu.CompilerParams(
            collective_id=0,
            disable_bounds_checks=True,
            disable_semaphore_checks=True,
        ),
    )(x, gamma)
```

```python
import jax
import jax.numpy as jnp
from jax import lax
from jax.experimental import pallas as pl
from jax.experimental.pallas import tpu as pltpu

N_DEV = 4
EPS = 1e-5
SUBLANES, LANES = 8, 128
NEAR = (1, 3)
FAR = 2

HEAD = (256, 128)
TAIL = (128, 112, 64, 40, 40)


def pallas_dist_rmsnorm_colshard_i_m768_n512_kernel(
    x: jax.Array,
    gamma: jax.Array,
):
    m, n = x.shape
    n_head, n_tail = sum(HEAD), len(TAIL)
    chunk_rows = HEAD + TAIL
    chunk_start = [sum(chunk_rows[:k]) for k in range(len(chunk_rows))]
    tail_start = chunk_start[len(HEAD):]
    assert sum(chunk_rows) == m and n % LANES == 0
    assert all(r % LANES == 0 for r in HEAD)
    assert all(r % SUBLANES == 0 and r <= LANES for r in TAIL)
    inv_cols = 1.0 / (n * N_DEV)
    tile = (SUBLANES, LANES)

    def body(
        x_hbm, g_hbm, out,
        xv, gv, head_own, head_in, tail_own, tail_near, tail_far, tail_base,
        load_sems, g_sem, send_sems, head_sem, near_sem, far_sems,
    ):
        loads = []
        for k, (r0, rows) in enumerate(zip(chunk_start, chunk_rows)):
            chunk = pl.ds(r0, rows)
            loads.append(
                pltpu.make_async_copy(x_hbm.at[chunk], xv.at[chunk], load_sems.at[k])
            )
            loads[-1].start()

        me = lax.axis_index("i")

        def peer(dist):
            return dict(
                device_id=((me + dist) & (N_DEV - 1),),
                device_id_type=pl.DeviceIdType.MESH,
            )

        barrier = pltpu.get_barrier_semaphore()
        for dist in (FAR, *NEAR):
            pl.semaphore_signal(barrier, 1, **peer(dist))

        g_load = pltpu.make_async_copy(g_hbm, gv, g_sem)
        g_load.start()

        sends = []

        def send(src, dst, recv_sem, dist):
            sends.append(
                pltpu.make_async_remote_copy(
                    src, dst, send_sems.at[len(sends)], recv_sem, **peer(dist)
                )
            )
            sends[-1].start()
            return sends[-1]

        sub = lax.broadcasted_iota(jnp.int32, tile, 0)
        skew = lax.broadcasted_iota(jnp.int32, tile, 1) - sub

        def packed_sumsq(r0, rows):
            acc = jnp.zeros(tile, jnp.float32)
            for l in range(0, rows, SUBLANES):
                v = xv[pl.ds(r0 + l, SUBLANES), :]
                v = v * v
                parts = [v[:, c : c + LANES] for c in range(0, n, LANES)]
                while len(parts) > 1:
                    parts = parts[2:] + [parts[0] + parts[1]]
                row_sum = jnp.sum(parts[0], axis=1, keepdims=True)
                acc = jnp.where(skew == l, row_sum, acc)
            return jnp.sum(acc, axis=0, keepdims=True)

        def unpack(packed, l):
            return jnp.sum(jnp.where(skew == l, packed, 0.0), axis=1, keepdims=True)

        def to_tile(v):
            return jnp.broadcast_to(v, tile)

        for k, rows in enumerate(HEAD):
            loads[k].wait()
            for r0 in range(chunk_start[k], chunk_start[k] + rows, LANES):
                head_own[pl.ds(r0 // LANES, 1), :] = packed_sumsq(r0, LANES)
        pl.semaphore_wait(barrier, N_DEV - 1)
        for dist in (FAR, *NEAR):
            send(head_own, head_in.at[dist - 1], head_sem, dist)
        far_copies = []
        for t, rows in enumerate(TAIL):
            loads[len(HEAD) + t].wait()
            tail_own[t] = packed_sumsq(tail_start[t], rows)
            far_copies.append(
                send(tail_own.at[t], tail_far.at[t], far_sems.at[t], FAR)
            )
        for slot, dist in enumerate(NEAR):
            send(tail_own, tail_near.at[slot], near_sem, dist)

        g_load.wait()
        g = jnp.broadcast_to(gv[...].reshape(1, n), (SUBLANES, n))
        for r0 in range(0, m, SUBLANES):
            xv[pl.ds(r0, SUBLANES), :] = xv[pl.ds(r0, SUBLANES), :] * g
        for copy in sends:
            copy.wait_send()

        pltpu.make_async_copy(head_in, head_in, head_sem).wait()
        for r0 in range(0, n_head, LANES):
            line = pl.ds(r0 // LANES, 1)
            total = (to_tile(head_own[line, :]) + to_tile(head_in[0, line, :])) + (
                to_tile(head_in[1, line, :]) + to_tile(head_in[2, line, :])
            )
            scale = lax.rsqrt(total * inv_cols + EPS)
            for l in range(0, LANES, SUBLANES):
                rows8 = pl.ds(r0 + l, SUBLANES)
                out[rows8, :] = xv[rows8, :] * unpack(scale, l)

        pltpu.make_async_copy(tail_near, tail_near, near_sem).wait()
        for t, rows in enumerate(TAIL):
            total = to_tile(tail_own[t]) + (
                to_tile(tail_near[0, t]) + to_tile(tail_near[1, t])
            )
            mean_eps = total * inv_cols + EPS
            for l in range(0, rows, SUBLANES):
                group = (tail_start[t] - n_head + l) // SUBLANES
                tail_base[group] = to_tile(unpack(mean_eps, l))

        for t, rows in enumerate(TAIL):
            far_copies[t].wait_recv()
            for l in range(0, rows, SUBLANES):
                far = jnp.full(tile, tail_far[t, 0, l], jnp.float32)
                for i in range(1, SUBLANES):
                    far = jnp.where(sub == i, tail_far[t, 0, l + i], far)
                group = (tail_start[t] - n_head + l) // SUBLANES
                scale = lax.rsqrt(tail_base[group] + far * inv_cols)
                rows8 = pl.ds(tail_start[t] + l, SUBLANES)
                out[rows8, :] = xv[rows8, :] * jnp.tile(scale, (1, n // LANES))

    f32 = jnp.float32
    return pl.pallas_call(
        body,
        out_shape=jax.ShapeDtypeStruct((m, n), x.dtype),
        in_specs=[pl.BlockSpec(memory_space=pltpu.HBM)] * 2,
        out_specs=pl.BlockSpec(memory_space=pltpu.VMEM),
        scratch_shapes=[
            pltpu.VMEM((m, n), f32),
            pltpu.VMEM((n,), f32),
            pltpu.VMEM((n_head // LANES, LANES), f32),
            pltpu.VMEM((N_DEV - 1, n_head // LANES, LANES), f32),
            pltpu.VMEM((n_tail, 1, LANES), f32),
            pltpu.VMEM((len(NEAR), n_tail, 1, LANES), f32),
            pltpu.SMEM((n_tail, 1, LANES), f32),
            pltpu.VMEM((sum(TAIL) // SUBLANES, *tile), f32),
            pltpu.SemaphoreType.DMA((len(chunk_rows),)),
            pltpu.SemaphoreType.DMA,
            pltpu.SemaphoreType.DMA((N_DEV - 1 + n_tail + len(NEAR),)),
            pltpu.SemaphoreType.DMA,
            pltpu.SemaphoreType.DMA,
            pltpu.SemaphoreType.DMA((n_tail,)),
        ],
        compiler_params=pltpu.CompilerParams(
            collective_id=0,
            disable_bounds_checks=True,
            disable_semaphore_checks=True,
        ),
    )(x, gamma)
```
